```python
import numpy as np

kernel_name = "dist_ring_attn_i_s256_d64"

def setup_inputs():
    S, D = 1024, 64
    q = np.random.randn(S, D).astype(np.float32)
    k = np.random.randn(S, D).astype(np.float32)
    v = np.random.randn(S, D).astype(np.float32)
    return {"q": q, "k": k, "v": v}

def reference(q: np.ndarray, k: np.ndarray, v: np.ndarray) -> np.ndarray:
    D = q.shape[1]
    scores = q @ k.T / np.sqrt(D)
    scores_max = np.max(scores, axis=1, keepdims=True)
    weights = np.exp(scores - scores_max)
    weights = weights / np.sum(weights, axis=1, keepdims=True)
    return weights @ v
```

```python
import jax
import jax.numpy as jnp
from jax import lax
from jax.experimental import pallas as pl
from jax.experimental.pallas import tpu as pltpu

N_DEV = 4
S_LOC = 256
D = 64
HALF = S_LOC // 2


def pallas_dist_ring_attn_i_s256_d64_kernel(q: jax.Array, k: jax.Array, v: jax.Array):
    def body(q_ref, k_ref, v_ref, o_ref, kv_buf, send_sems, recv_sems):
        me = lax.axis_index("i")
        left = lax.rem(me + N_DEV - 1, N_DEV)
        right = lax.rem(me + 1, N_DEV)

        barrier = pltpu.get_barrier_semaphore()
        for nbr in (left, right):
            pl.semaphore_signal(barrier, inc=1, device_id=(nbr,),
                                device_id_type=pl.DeviceIdType.MESH)

        kv_buf[0, :, 0:D] = k_ref[...].astype(jnp.bfloat16)
        kv_buf[0, :, D:2 * D] = v_ref[...].astype(jnp.bfloat16)

        pl.semaphore_wait(barrier, 2)

        def copy(idx, src_slot, dst_slot, half, dev):
            rows = pl.ds(half * HALF, HALF)
            return pltpu.make_async_remote_copy(
                src_ref=kv_buf.at[src_slot, rows],
                dst_ref=kv_buf.at[dst_slot, rows],
                send_sem=send_sems.at[idx],
                recv_sem=recv_sems.at[idx],
                device_id=(dev,),
                device_id_type=pl.DeviceIdType.MESH,
            )

        c_rA = copy(0, 0, 1, 0, right)
        c_lB = copy(1, 0, 2, 1, left)
        c_rB = copy(2, 0, 1, 1, right)
        c_lA = copy(3, 0, 2, 0, left)
        f_r = copy(4, 1, 3, 0, right)
        f_l = copy(5, 2, 3, 1, left)
        c_rA.start()
        c_lB.start()
        c_rB.start()
        c_lA.start()

        qs = q_ref[...] * jnp.float32(0.125)
        qp = jnp.concatenate([qs, jnp.zeros_like(qs)], axis=1).astype(jnp.bfloat16)

        def chunk(slot, half):
            kvc = kv_buf[slot, pl.ds(half * HALF, HALF), :]
            s = lax.dot_general(qp, kvc, (((1,), (1,)), ((), ())),
                                preferred_element_type=jnp.float32)
            m = jnp.max(s, axis=1, keepdims=True)
            p = jnp.exp(s - m)
            l = jnp.sum(p, axis=1, keepdims=True)
            o = jnp.dot(p.astype(jnp.bfloat16), kvc, preferred_element_type=jnp.float32)
            return m, l, o

        parts = [chunk(0, 0), chunk(0, 1)]
        c_rA.wait_recv()
        f_r.start()
        c_lB.wait_recv()
        f_l.start()
        parts.append(chunk(1, 0))
        parts.append(chunk(2, 1))
        c_rB.wait_recv()
        parts.append(chunk(1, 1))
        c_lA.wait_recv()
        parts.append(chunk(2, 0))
        f_r.wait_recv()
        parts.append(chunk(3, 0))
        f_l.wait_recv()
        parts.append(chunk(3, 1))

        m = parts[0][0]
        for pt in parts[1:]:
            m = jnp.maximum(m, pt[0])
        l = jnp.zeros_like(m)
        o = jnp.zeros((S_LOC, 2 * D), jnp.float32)
        for (mc, lc, oc) in parts:
            a = jnp.exp(mc - m)
            l = l + a * lc
            o = o + a * oc
        o_ref[...] = (o / l)[:, D:2 * D]

        for c in (c_rA, c_lB, c_rB, c_lA, f_r, f_l):
            c.wait_send()

    return pl.pallas_call(
        body,
        out_shape=jax.ShapeDtypeStruct((S_LOC, D), jnp.float32),
        in_specs=[pl.BlockSpec(memory_space=pltpu.VMEM)] * 3,
        out_specs=pl.BlockSpec(memory_space=pltpu.VMEM),
        scratch_shapes=[
            pltpu.VMEM((N_DEV, S_LOC, 2 * D), jnp.bfloat16),
            pltpu.SemaphoreType.DMA((6,)),
            pltpu.SemaphoreType.DMA((6,)),
        ],
        compiler_params=pltpu.CompilerParams(collective_id=0),
    )(q, k, v)
```

```python
import jax
import jax.numpy as jnp
from jax import lax
from jax.experimental import pallas as pl
from jax.experimental.pallas import tpu as pltpu

N_DEV = 4
S_LOC = 256
D = 64
HK = 128


def pallas_dist_ring_attn_i_s256_d64_kernel(q: jax.Array, k: jax.Array, v: jax.Array):
    qT, kT, vT = q.T, k.T, v.T

    def body(q_hbm, k_hbm, v_hbm, o_hbm, q_v, k_v, v_v, o_v, buf, in_sems, out_sem,
             send_sems, recv_sems):
        me = lax.axis_index("i")
        left = lax.rem(me + N_DEV - 1, N_DEV)
        right = lax.rem(me + 1, N_DEV)

        barrier = pltpu.get_barrier_semaphore()
        for nbr in (left, right):
            pl.semaphore_signal(barrier, inc=1, device_id=(nbr,),
                                device_id_type=pl.DeviceIdType.MESH)

        ck = pltpu.make_async_copy(k_hbm, k_v, in_sems.at[0])
        cv = pltpu.make_async_copy(v_hbm, v_v, in_sems.at[1])
        cq = pltpu.make_async_copy(q_hbm, q_v, in_sems.at[2])
        ck.start()
        cv.start()
        cq.start()

        ck.wait()
        buf[0, 0] = k_v[:, 0:HK].astype(jnp.bfloat16)
        buf[0, 2] = k_v[:, HK:2 * HK].astype(jnp.bfloat16)
        cv.wait()
        buf[0, 1] = v_v[:, 0:HK].astype(jnp.bfloat16)
        buf[0, 3] = v_v[:, HK:2 * HK].astype(jnp.bfloat16)

        pl.semaphore_wait(barrier, 2)

        def copy(idx, src_slot, dst_slot, piece, dev):
            return pltpu.make_async_remote_copy(
                src_ref=buf.at[src_slot, piece],
                dst_ref=buf.at[dst_slot, piece],
                send_sem=send_sems.at[idx],
                recv_sem=recv_sems.at[idx],
                device_id=(dev,),
                device_id_type=pl.DeviceIdType.MESH,
            )

        to_r = [copy(c, 0, 1, c, right) for c in range(4)]
        to_l = [copy(4 + c, 0, 2, c, left) for c in range(4)]
        fw_r = [copy(8 + c, 1, 3, c, right) for c in (0, 1)]
        fw_l = [copy(8 + c, 2, 3, c, left) for c in (2, 3)]
        to_r[0].start(); to_l[2].start()
        to_r[1].start(); to_l[3].start()
        to_r[2].start(); to_l[0].start()
        to_r[3].start(); to_l[1].start()

        cq.wait()
        qb = (q_v[...] * jnp.float32(0.125)).astype(jnp.bfloat16)

        def scores(slot, h):
            kc = buf[slot, 2 * h]
            s = lax.dot_general(kc, qb, (((0,), (0,)), ((), ())),
                                preferred_element_type=jnp.float32)
            m = jnp.max(s, axis=0, keepdims=True)
            p = jnp.exp(s - m)
            l = jnp.sum(p, axis=0, keepdims=True)
            return m, l, p.astype(jnp.bfloat16)

        def pv(slot, h, p):
            return jnp.dot(buf[slot, 2 * h + 1], p, preferred_element_type=jnp.float32)

        parts = []
        for h in range(2):
            m, l, p = scores(0, h)
            parts.append((m, l, pv(0, h, p)))

        to_r[0].wait_recv(); fw_r[0].start()
        to_l[2].wait_recv(); fw_l[0].start()
        to_r[1].wait_recv(); fw_r[1].start()
        to_l[3].wait_recv(); fw_l[1].start()

        m, l, p = scores(1, 0)
        parts.append((m, l, pv(1, 0, p)))
        m, l, p = scores(2, 1)
        parts.append((m, l, pv(2, 1, p)))

        to_r[2].wait_recv()
        m, l, p = scores(1, 1)
        to_r[3].wait_recv()
        parts.append((m, l, pv(1, 1, p)))
        to_l[0].wait_recv()
        m, l, p = scores(2, 0)
        to_l[1].wait_recv()
        parts.append((m, l, pv(2, 0, p)))

        fw_r[0].wait_recv()
        m, l, p = scores(3, 0)
        fw_l[0].wait_recv()
        m2, l2, p2 = scores(3, 1)
        fw_r[1].wait_recv()
        parts.append((m, l, pv(3, 0, p)))
        fw_l[1].wait_recv()
        parts.append((m2, l2, pv(3, 1, p2)))

        m = parts[0][0]
        for pt in parts[1:]:
            m = jnp.maximum(m, pt[0])
        l = jnp.zeros_like(m)
        o = jnp.zeros((D, S_LOC), jnp.float32)
        for (mc, lc, oc) in parts:
            a = jnp.exp(mc - m)
            l = l + a * lc
            o = o + a * oc
        o_v[...] = o / l
        co = pltpu.make_async_copy(o_v, o_hbm, out_sem)
        co.start()

        for c in to_r + to_l + fw_r + fw_l:
            c.wait_send()
        co.wait()

    oT = pl.pallas_call(
        body,
        out_shape=jax.ShapeDtypeStruct((D, S_LOC), jnp.float32),
        in_specs=[pl.BlockSpec(memory_space=pl.ANY)] * 3,
        out_specs=pl.BlockSpec(memory_space=pl.ANY),
        scratch_shapes=[
            pltpu.VMEM((D, S_LOC), jnp.float32),
            pltpu.VMEM((D, S_LOC), jnp.float32),
            pltpu.VMEM((D, S_LOC), jnp.float32),
            pltpu.VMEM((D, S_LOC), jnp.float32),
            pltpu.VMEM((N_DEV, 4, D, HK), jnp.bfloat16),
            pltpu.SemaphoreType.DMA((3,)),
            pltpu.SemaphoreType.DMA,
            pltpu.SemaphoreType.DMA((12,)),
            pltpu.SemaphoreType.DMA((12,)),
        ],
        compiler_params=pltpu.CompilerParams(collective_id=0),
    )(qT, kT, vT)
    return oT.T
```

```python
import jax
import jax.numpy as jnp
from jax import lax
from jax.experimental import pallas as pl
from jax.experimental.pallas import tpu as pltpu

N_DEV = 4
S_LOC = 256
D = 64
HK = 128


def pallas_dist_ring_attn_i_s256_d64_kernel(q: jax.Array, k: jax.Array, v: jax.Array):
    qT, kT, vT = q.T, k.T, v.T

    def body(q_hbm, k_hbm, v_hbm, o_ref, q_v, k_v, v_v, buf, in_sems,
             send_sems, recv_sems):
        me = lax.axis_index("i")
        left = lax.rem(me + N_DEV - 1, N_DEV)
        right = lax.rem(me + 1, N_DEV)

        barrier = pltpu.get_barrier_semaphore()
        for nbr in (left, right):
            pl.semaphore_signal(barrier, inc=1, device_id=(nbr,),
                                device_id_type=pl.DeviceIdType.MESH)

        ck = pltpu.make_async_copy(k_hbm, k_v, in_sems.at[0])
        cv = pltpu.make_async_copy(v_hbm, v_v, in_sems.at[1])
        cq = pltpu.make_async_copy(q_hbm, q_v, in_sems.at[2])
        ck.start()
        cv.start()
        cq.start()

        ck.wait()
        buf[0, 0] = k_v[:, 0:HK].astype(jnp.bfloat16)
        buf[0, 2] = k_v[:, HK:2 * HK].astype(jnp.bfloat16)
        cv.wait()
        buf[0, 1] = v_v[:, 0:HK].astype(jnp.bfloat16)
        buf[0, 3] = v_v[:, HK:2 * HK].astype(jnp.bfloat16)

        pl.semaphore_wait(barrier, 2)

        def copy(idx, src_slot, dst_slot, piece, dev):
            return pltpu.make_async_remote_copy(
                src_ref=buf.at[src_slot, piece],
                dst_ref=buf.at[dst_slot, piece],
                send_sem=send_sems.at[idx],
                recv_sem=recv_sems.at[idx],
                device_id=(dev,),
                device_id_type=pl.DeviceIdType.MESH,
            )

        to_r = [copy(c, 0, 1, c, right) for c in range(4)]
        to_l = [copy(4 + c, 0, 2, c, left) for c in range(4)]
        fw_r = [copy(8 + c, 1, 3, c, right) for c in (0, 1)]
        fw_l = [copy(8 + c, 2, 3, c, left) for c in (2, 3)]
        to_r[0].start(); to_l[2].start()
        to_r[1].start(); to_l[3].start()
        to_r[2].start(); to_l[0].start()
        to_r[3].start(); to_l[1].start()

        cq.wait()
        qb = (q_v[...] * jnp.float32(0.125)).astype(jnp.bfloat16)

        def scores(slot, h):
            kc = buf[slot, 2 * h]
            return lax.dot_general(kc, qb, (((0,), (0,)), ((), ())),
                                   preferred_element_type=jnp.float32)

        def pv(slot, h, p):
            return jnp.dot(buf[slot, 2 * h + 1], p, preferred_element_type=jnp.float32)

        def pair(state, c0, c1, wait_v=None):
            s0 = scores(*c0)
            s1 = scores(*c1)
            mc = jnp.maximum(jnp.max(s0, axis=0, keepdims=True),
                             jnp.max(s1, axis=0, keepdims=True))
            if state is not None:
                m, l, o = state
                mn = jnp.maximum(m, mc)
                a = jnp.exp(m - mn)
            else:
                mn = mc
            p0 = jnp.exp(s0 - mn)
            p1 = jnp.exp(s1 - mn)
            ls = jnp.sum(p0, axis=0, keepdims=True) + jnp.sum(p1, axis=0, keepdims=True)
            p0 = p0.astype(jnp.bfloat16)
            p1 = p1.astype(jnp.bfloat16)
            if state is not None:
                ln = a * l + ls
                ob = a * o
            else:
                ln = ls
                ob = None
            if wait_v is not None:
                wait_v()
            on = pv(*c0, p0) + pv(*c1, p1)
            if ob is not None:
                on = on + ob
            return mn, ln, on

        st = pair(None, (0, 0), (0, 1))

        to_r[0].wait_recv(); fw_r[0].start()
        to_l[2].wait_recv(); fw_l[0].start()
        to_r[1].wait_recv(); fw_r[1].start()
        to_l[3].wait_recv(); fw_l[1].start()

        st = pair(st, (1, 0), (2, 1))

        to_r[2].wait_recv()
        to_l[0].wait_recv()

        def wv1():
            to_r[3].wait_recv()
            to_l[1].wait_recv()
        st = pair(st, (1, 1), (2, 0), wv1)

        fw_r[0].wait_recv()
        fw_l[0].wait_recv()

        def wv2():
            fw_r[1].wait_recv()
            fw_l[1].wait_recv()
        m, l, o = pair(st, (3, 0), (3, 1), wv2)
        o_ref[...] = o / l

        for c in to_r + to_l + fw_r + fw_l:
            c.wait_send()

    oT = pl.pallas_call(
        body,
        out_shape=jax.ShapeDtypeStruct((D, S_LOC), jnp.float32),
        in_specs=[pl.BlockSpec(memory_space=pl.ANY)] * 3,
        out_specs=pl.BlockSpec(memory_space=pltpu.VMEM),
        scratch_shapes=[
            pltpu.VMEM((D, S_LOC), jnp.float32),
            pltpu.VMEM((D, S_LOC), jnp.float32),
            pltpu.VMEM((D, S_LOC), jnp.float32),
            pltpu.VMEM((N_DEV, 4, D, HK), jnp.bfloat16),
            pltpu.SemaphoreType.DMA((3,)),
            pltpu.SemaphoreType.DMA((12,)),
            pltpu.SemaphoreType.DMA((12,)),
        ],
        compiler_params=pltpu.CompilerParams(collective_id=0),
    )(qT, kT, vT)
    return oT.T
```

```python
import jax
import jax.numpy as jnp
from jax import lax
from jax.experimental import pallas as pl
from jax.experimental.pallas import tpu as pltpu

N_DEV = 4
S_LOC = 256
D = 64
HK = 128


def pallas_dist_ring_attn_i_s256_d64_kernel(q: jax.Array, k: jax.Array, v: jax.Array):
    qT, kT, vT = q.T, k.T, v.T

    def body(q_hbm, k_hbm, v_hbm, o_ref, q_v, k_v, v_v, buf, in_sems,
             send_sems, recv_sems, ack_sems):
        me = lax.axis_index("i")
        left = lax.rem(me + N_DEV - 1, N_DEV)
        right = lax.rem(me + 1, N_DEV)
        diag = lax.rem(me + 2, N_DEV)
        is0, is1, is2, is3 = (me == 0), (me == 1), (me == 2), (me == 3)

        barrier = pltpu.get_barrier_semaphore()

        def bsig(dev):
            pl.semaphore_signal(barrier, inc=1, device_id=(dev,),
                                device_id_type=pl.DeviceIdType.MESH)

        def ack(dev, which):
            pl.semaphore_signal(ack_sems.at[which], inc=1, device_id=(dev,),
                                device_id_type=pl.DeviceIdType.MESH)

        @pl.when(is0)
        def _():
            bsig(left)
            bsig(right)
            bsig(diag)

        @pl.when(is1)
        def _():
            bsig(right)

        @pl.when(is3)
        def _():
            bsig(left)

        ck = pltpu.make_async_copy(k_hbm, k_v, in_sems.at[0])
        cv = pltpu.make_async_copy(v_hbm, v_v, in_sems.at[1])
        cq = pltpu.make_async_copy(q_hbm, q_v, in_sems.at[2])
        ck.start()
        cv.start()
        cq.start()

        @pl.when(is1)
        def _():
            pl.semaphore_wait(barrier, 1)
            ack(left, 1)

        @pl.when(is3)
        def _():
            pl.semaphore_wait(barrier, 1)
            ack(right, 0)

        @pl.when(is2)
        def _():
            pl.semaphore_wait(barrier, 3)
            ack(left, 1)
            ack(right, 0)

        def cp(src_slot, dst_slot, piece, dev, ssem):
            return pltpu.make_async_remote_copy(
                src_ref=buf.at[src_slot, piece], dst_ref=buf.at[dst_slot, piece],
                send_sem=send_sems.at[ssem],
                recv_sem=recv_sems.at[(dst_slot - 1) * 4 + piece],
                device_id=(dev,), device_id_type=pl.DeviceIdType.MESH)

        to_r = [cp(0, 1, c, right, c) for c in range(4)]
        to_l = [cp(0, 2, c, left, 4 + c) for c in range(4)]
        fw_r = [cp(1, 3, c, right, 8 + c) for c in range(4)]
        fw_l = [None, None] + [cp(2, 3, c, left, 10 + c) for c in (2, 3)]
        to_d = {c: cp(0, 3, c, diag, 14 + c) for c in (0, 2, 3)}

        ck.wait()
        buf[0, 0] = k_v[:, 0:HK].astype(jnp.bfloat16)
        buf[0, 2] = k_v[:, HK:2 * HK].astype(jnp.bfloat16)

        @pl.when(is2)
        def _():
            to_d[0].start()
            to_d[2].start()

        cv.wait()
        buf[0, 1] = v_v[:, 0:HK].astype(jnp.bfloat16)
        buf[0, 3] = v_v[:, HK:2 * HK].astype(jnp.bfloat16)

        def send_r():
            for c in (0, 1, 2, 3):
                to_r[c].start()

        def send_l():
            for c in (2, 3, 0, 1):
                to_l[c].start()

        @pl.when(is2)
        def _():
            to_r[1].start()
            to_d[3].start()
            to_r[0].start(); to_l[2].start()
            to_r[2].start(); to_l[3].start()
            to_r[3].start(); to_l[0].start()
            to_l[1].start()

        pl.when(is1)(send_l)
        pl.when(is3)(send_r)

        cq.wait()
        qb = (q_v[...] * jnp.float32(0.125)).astype(jnp.bfloat16)

        def scores(slot, h):
            kc = buf[slot, 2 * h]
            return lax.dot_general(kc, qb, (((0,), (0,)), ((), ())),
                                   preferred_element_type=jnp.float32)

        def pv(slot, h, p):
            return jnp.dot(buf[slot, 2 * h + 1], p, preferred_element_type=jnp.float32)

        def pair(state, c0, c1, wait_v=None):
            s0 = scores(*c0)
            s1 = scores(*c1)
            mc = jnp.maximum(jnp.max(s0, axis=0, keepdims=True),
                             jnp.max(s1, axis=0, keepdims=True))
            if state is not None:
                m, l, o = state
                mn = jnp.maximum(m, mc)
                a = jnp.exp(m - mn)
            else:
                mn = mc
            p0 = jnp.exp(s0 - mn)
            p1 = jnp.exp(s1 - mn)
            ls = jnp.sum(p0, axis=0, keepdims=True) + jnp.sum(p1, axis=0, keepdims=True)
            p0 = p0.astype(jnp.bfloat16)
            p1 = p1.astype(jnp.bfloat16)
            if state is not None:
                ln = a * l + ls
                ob = a * o
            else:
                ln = ls
                ob = None
            if wait_v is not None:
                wait_v()
            on = pv(*c0, p0) + pv(*c1, p1)
            if ob is not None:
                on = on + ob
            return mn, ln, on

        st = pair(None, (0, 0), (0, 1))

        @pl.when(jnp.logical_or(is0, is3))
        def _():
            pl.semaphore_wait(ack_sems.at[0], 1)
            send_l()

        @pl.when(jnp.logical_or(is0, is1))
        def _():
            pl.semaphore_wait(ack_sems.at[1], 1)
            send_r()

        @pl.when(is0)
        def _():
            to_r[0].wait_recv(); fw_r[0].start()
            to_l[2].wait_recv(); fw_l[2].start()
            to_r[1].wait_recv(); fw_r[1].start()
            to_l[3].wait_recv(); fw_l[3].start()

        @pl.when(jnp.logical_or(is1, is2))
        def _():
            to_r[0].wait_recv(); fw_r[0].start()
            to_r[1].wait_recv(); fw_r[1].start()
            to_l[2].wait_recv()
            to_l[3].wait_recv()

        @pl.when(is3)
        def _():
            to_r[1].wait_recv(); fw_r[1].start()
            to_l[2].wait_recv(); fw_l[2].start()
            to_l[3].wait_recv(); fw_l[3].start()
            to_r[0].wait_recv()

        st = pair(st, (1, 0), (2, 1))

        to_r[2].wait_recv()
        pl.when(is0)(fw_r[2].start)
        to_l[0].wait_recv()

        def wv1():
            to_r[3].wait_recv()
            pl.when(is0)(fw_r[3].start)
            to_l[1].wait_recv()
        st = pair(st, (1, 1), (2, 0), wv1)

        fw_r[0].wait_recv()
        fw_l[2].wait_recv()

        def wv2():
            fw_r[1].wait_recv()
            fw_l[3].wait_recv()
        m, l, o = pair(st, (3, 0), (3, 1), wv2)
        o_ref[...] = o / l

        for c in to_r + to_l + [fw_r[1]]:
            c.wait_send()

        @pl.when(is0)
        def _():
            for c in [fw_r[0], fw_r[2], fw_r[3]] + fw_l[2:]:
                c.wait_send()

        @pl.when(is1)
        def _():
            fw_r[0].wait_send()

        @pl.when(is2)
        def _():
            for c in [to_d[0], to_d[2], to_d[3], fw_r[0]]:
                c.wait_send()

        @pl.when(is3)
        def _():
            for c in fw_l[2:]:
                c.wait_send()

    oT = pl.pallas_call(
        body,
        out_shape=jax.ShapeDtypeStruct((D, S_LOC), jnp.float32),
        in_specs=[pl.BlockSpec(memory_space=pl.ANY)] * 3,
        out_specs=pl.BlockSpec(memory_space=pltpu.VMEM),
        scratch_shapes=[
            pltpu.VMEM((D, S_LOC), jnp.float32),
            pltpu.VMEM((D, S_LOC), jnp.float32),
            pltpu.VMEM((D, S_LOC), jnp.float32),
            pltpu.VMEM((N_DEV, 4, D, HK), jnp.bfloat16),
            pltpu.SemaphoreType.DMA((3,)),
            pltpu.SemaphoreType.DMA((18,)),
            pltpu.SemaphoreType.DMA((12,)),
            pltpu.SemaphoreType.REGULAR((2,)),
        ],
        compiler_params=pltpu.CompilerParams(collective_id=0),
    )(qT, kT, vT)
    return oT.T
```

```python
import jax
import jax.numpy as jnp
from jax import lax
from jax.experimental import pallas as pl
from jax.experimental.pallas import tpu as pltpu

N_DEV = 4
S_LOC = 256
D = 64
HK = 128


def pallas_dist_ring_attn_i_s256_d64_kernel(q: jax.Array, k: jax.Array, v: jax.Array):
    qT, kT, vT = q.T, k.T, v.T

    def body(q_hbm, k_hbm, v_hbm, o_ref, q_v, k_v, v_v, buf, kf, in_sems,
             send_sems, recv_sems, ack_sems):
        me = lax.axis_index("i")
        left = lax.rem(me + N_DEV - 1, N_DEV)
        right = lax.rem(me + 1, N_DEV)
        diag = lax.rem(me + 2, N_DEV)
        is0, is1, is2, is3 = (me == 0), (me == 1), (me == 2), (me == 3)

        barrier = pltpu.get_barrier_semaphore()

        def bsig(dev):
            pl.semaphore_signal(barrier, inc=1, device_id=(dev,),
                                device_id_type=pl.DeviceIdType.MESH)

        def ack(dev, which):
            pl.semaphore_signal(ack_sems.at[which], inc=1, device_id=(dev,),
                                device_id_type=pl.DeviceIdType.MESH)

        @pl.when(is0)
        def _():
            bsig(left)
            bsig(right)
            bsig(diag)

        @pl.when(is1)
        def _():
            bsig(right)

        @pl.when(is3)
        def _():
            bsig(left)

        early = pltpu.make_async_remote_copy(
            src_ref=k_hbm.at[:, pl.ds(HK, HK)], dst_ref=kf,
            send_sem=send_sems.at[15], recv_sem=recv_sems.at[12],
            device_id=(left,), device_id_type=pl.DeviceIdType.MESH)

        @pl.when(is1)
        def _():
            pl.semaphore_wait(barrier, 1)
            early.start()
            ack(left, 1)

        ck = pltpu.make_async_copy(k_hbm, k_v, in_sems.at[0])
        cv = pltpu.make_async_copy(v_hbm, v_v, in_sems.at[1])
        cq = pltpu.make_async_copy(q_hbm, q_v, in_sems.at[2])
        ck.start()
        cv.start()
        cq.start()

        @pl.when(is3)
        def _():
            pl.semaphore_wait(barrier, 1)
            ack(right, 0)

        @pl.when(is2)
        def _():
            pl.semaphore_wait(barrier, 3)
            ack(left, 1)
            ack(right, 0)

        def cp(src_slot, dst_slot, piece, dev, ssem):
            return pltpu.make_async_remote_copy(
                src_ref=buf.at[src_slot, piece], dst_ref=buf.at[dst_slot, piece],
                send_sem=send_sems.at[ssem],
                recv_sem=recv_sems.at[(dst_slot - 1) * 4 + piece],
                device_id=(dev,), device_id_type=pl.DeviceIdType.MESH)

        to_r = [cp(0, 1, c, right, c) for c in range(4)]
        to_l = [cp(0, 2, c, left, 4 + c) for c in range(4)]
        fw_r = [cp(1, 3, c, right, 8 + c) for c in range(4)]
        fw_l = [None, None] + [cp(2, 3, c, left, 10 + c) for c in (2, 3)]
        to_d = {c: cp(0, 3, c, diag, 14 + c) for c in (0, 2, 3)}

        ck.wait()
        buf[0, 0] = k_v[:, 0:HK].astype(jnp.bfloat16)
        buf[0, 2] = k_v[:, HK:2 * HK].astype(jnp.bfloat16)

        @pl.when(is2)
        def _():
            to_d[0].start()
            to_d[2].start()

        cv.wait()
        buf[0, 1] = v_v[:, 0:HK].astype(jnp.bfloat16)
        buf[0, 3] = v_v[:, HK:2 * HK].astype(jnp.bfloat16)

        def send_r():
            for c in (0, 1, 2, 3):
                to_r[c].start()

        def send_l():
            for c in (2, 3, 0, 1):
                to_l[c].start()

        @pl.when(is2)
        def _():
            to_r[1].start()
            to_d[3].start()
            to_r[0].start(); to_l[2].start()
            to_r[2].start(); to_l[3].start()
            to_r[3].start(); to_l[0].start()
            to_l[1].start()

        @pl.when(is1)
        def _():
            for c in (3, 0, 1):
                to_l[c].start()
        pl.when(is3)(send_r)

        cq.wait()
        qb = (q_v[...] * jnp.float32(0.125)).astype(jnp.bfloat16)

        def scores(slot, h):
            kc = buf[slot, 2 * h]
            return lax.dot_general(kc, qb, (((0,), (0,)), ((), ())),
                                   preferred_element_type=jnp.float32)

        def pv(slot, h, p):
            return jnp.dot(buf[slot, 2 * h + 1], p, preferred_element_type=jnp.float32)

        def pair(state, c0, c1, wait_v=None):
            s0 = scores(*c0)
            s1 = scores(*c1)
            mc = jnp.maximum(jnp.max(s0, axis=0, keepdims=True),
                             jnp.max(s1, axis=0, keepdims=True))
            if state is not None:
                m, l, o = state
                mn = jnp.maximum(m, mc)
                a = jnp.exp(m - mn)
            else:
                mn = mc
            p0 = jnp.exp(s0 - mn)
            p1 = jnp.exp(s1 - mn)
            ls = jnp.sum(p0, axis=0, keepdims=True) + jnp.sum(p1, axis=0, keepdims=True)
            p0 = p0.astype(jnp.bfloat16)
            p1 = p1.astype(jnp.bfloat16)
            if state is not None:
                ln = a * l + ls
                ob = a * o
            else:
                ln = ls
                ob = None
            if wait_v is not None:
                wait_v()
            on = pv(*c0, p0) + pv(*c1, p1)
            if ob is not None:
                on = on + ob
            return mn, ln, on

        st = pair(None, (0, 0), (0, 1))

        @pl.when(jnp.logical_or(is0, is3))
        def _():
            pl.semaphore_wait(ack_sems.at[0], 1)
            send_l()

        @pl.when(jnp.logical_or(is0, is1))
        def _():
            pl.semaphore_wait(ack_sems.at[1], 1)
            send_r()

        st0 = st

        @pl.when(is1)
        def _():
            to_r[0].wait_recv(); fw_r[0].start()
            to_r[1].wait_recv(); fw_r[1].start()
            to_r[2].wait_recv()
            st = pair(st0, (1, 0), (1, 1), to_r[3].wait_recv)
            fw_r[0].wait_recv()
            to_l[2].wait_recv()

            def wa():
                fw_r[1].wait_recv()
                to_l[3].wait_recv()
            st = pair(st, (3, 0), (2, 1), wa)
            fw_l[2].wait_recv()
            to_l[0].wait_recv()

            def wb():
                fw_l[3].wait_recv()
                to_l[1].wait_recv()
            m, l, o = pair(st, (3, 1), (2, 0), wb)
            o_ref[...] = o / l

        @pl.when(jnp.logical_not(is1))
        def _():
            @pl.when(is0)
            def _():
                early.wait_recv()
                buf[2, 2] = kf[...].astype(jnp.bfloat16)
                fw_l[2].start()
                to_r[0].wait_recv(); fw_r[0].start()
                to_r[1].wait_recv(); fw_r[1].start()
                to_l[3].wait_recv(); fw_l[3].start()

            @pl.when(is2)
            def _():
                to_r[0].wait_recv(); fw_r[0].start()
                to_r[1].wait_recv(); fw_r[1].start()
                to_l[2].wait_recv()
                to_l[3].wait_recv()

            @pl.when(is3)
            def _():
                to_r[1].wait_recv(); fw_r[1].start()
                to_l[2].wait_recv(); fw_l[2].start()
                to_l[3].wait_recv(); fw_l[3].start()
                to_r[0].wait_recv()

            st = pair(st0, (1, 0), (2, 1))

            to_r[2].wait_recv()
            pl.when(is0)(fw_r[2].start)
            to_l[0].wait_recv()

            def wv1():
                to_r[3].wait_recv()
                pl.when(is0)(fw_r[3].start)
                to_l[1].wait_recv()
            st = pair(st, (1, 1), (2, 0), wv1)

            fw_r[0].wait_recv()
            fw_l[2].wait_recv()

            def wv2():
                fw_r[1].wait_recv()
                fw_l[3].wait_recv()
            m, l, o = pair(st, (3, 0), (3, 1), wv2)
            o_ref[...] = o / l

        for c in to_r + [to_l[0], to_l[1], to_l[3], fw_r[1]]:
            c.wait_send()
        pl.when(jnp.logical_not(is1))(to_l[2].wait_send)

        @pl.when(is0)
        def _():
            for c in [fw_r[0], fw_r[2], fw_r[3]] + fw_l[2:]:
                c.wait_send()

        @pl.when(is1)
        def _():
            fw_r[0].wait_send()
            early.wait_send()

        @pl.when(is2)
        def _():
            for c in [to_d[0], to_d[2], to_d[3], fw_r[0]]:
                c.wait_send()

        @pl.when(is3)
        def _():
            for c in fw_l[2:]:
                c.wait_send()

    oT = pl.pallas_call(
        body,
        out_shape=jax.ShapeDtypeStruct((D, S_LOC), jnp.float32),
        in_specs=[pl.BlockSpec(memory_space=pl.ANY)] * 3,
        out_specs=pl.BlockSpec(memory_space=pltpu.VMEM),
        scratch_shapes=[
            pltpu.VMEM((D, S_LOC), jnp.float32),
            pltpu.VMEM((D, S_LOC), jnp.float32),
            pltpu.VMEM((D, S_LOC), jnp.float32),
            pltpu.VMEM((N_DEV, 4, D, HK), jnp.bfloat16),
            pltpu.VMEM((D, HK), jnp.float32),
            pltpu.SemaphoreType.DMA((3,)),
            pltpu.SemaphoreType.DMA((18,)),
            pltpu.SemaphoreType.DMA((13,)),
            pltpu.SemaphoreType.REGULAR((2,)),
        ],
        compiler_params=pltpu.CompilerParams(collective_id=0),
    )(qT, kT, vT)
    return oT.T
```
